```python
import numpy as np

kernel_name = "dist_moe_top2_ep_n1024_d512_e4_h1024"

def setup_inputs():
    x = np.random.randn(1024, 512).astype(np.float32)
    router_W = np.random.randn(512, 16).astype(np.float32) * 0.1
    scores64 = x.astype(np.float64) @ router_W.astype(np.float64)
    route_idx = np.argsort(-scores64, axis=-1)[:, :2].astype(np.int32)
    expert_W = np.random.randn(16, 512, 1024).astype(np.float32) * 0.02
    return {"x": x, "router_W": router_W, "route_idx": route_idx, "expert_W": expert_W}

def reference(x, router_W, route_idx, expert_W):
    scores = x @ router_W
    s_max = scores.max(axis=-1, keepdims=True)
    probs = np.exp(scores - s_max)
    probs = probs / probs.sum(axis=-1, keepdims=True)
    out = np.zeros((1024, 1024), dtype=np.float32)
    for i in range(1024):
        e0, e1 = int(route_idx[i, 0]), int(route_idx[i, 1])
        g0, g1 = probs[i, e0], probs[i, e1]
        gs = g0 + g1
        out[i] = (g0 / gs) * (x[i] @ expert_W[e0]) + (g1 / gs) * (x[i] @ expert_W[e1])
    return out
```

```python
import functools

import jax
import jax.numpy as jnp
from jax import lax
from jax.experimental import pallas as pl
from jax.experimental.pallas import tpu as pltpu

N_TOK, D_IN, D_OUT = 1024, 512, 1024
N_DEV, E_LOC, N_EXP = 4, 4, 16
NB, TB, HS = 4, 256, 64
NC, CW = 8, 128
WIN = 64
BF16, F32, I32 = jnp.bfloat16, jnp.float32, jnp.int32
MESH = pl.DeviceIdType.MESH

DEFAULT = dict(cap=176, base=96, gran=4, f0=128, scopes=False, loop=True)


def _dot(a, b):
    return jnp.dot(a, b, preferred_element_type=F32)


def _dot_nt(a, b):
    return lax.dot_general(a, b, (((1,), (1,)), ((), ())), preferred_element_type=F32)


def _iota(shape, dim):
    return lax.broadcasted_iota(I32, shape, dim)


def _count(flags):
    tri = jnp.where(_iota((128, 256), 0) < _iota((128, 256), 1), 1.0, 0.0).astype(BF16)
    lhs = jnp.concatenate([jnp.where(f, 1.0, 0.0) for f in flags], axis=0).astype(BF16)
    r = _dot(lhs, tri).astype(I32)
    return ([r[8 * k:8 * k + 8, :128] for k in range(len(flags))],
            [r[8 * k:8 * k + 8, 128:] for k in range(len(flags))])


def _pick(idx, vals):
    out = vals[-1]
    for k in range(len(vals) - 2, -1, -1):
        out = jnp.where(idx == k, vals[k], out)
    return out


def _block_lanes(v, b):
    return jnp.concatenate([v[2 * b:2 * b + 1], v[2 * b + 1:2 * b + 2]], axis=1)


def _body(cfg, x_hbm, rw_hbm, ri_hbm, w_hbm, out_ref,
          xv, rwv, riv, wv, xg, gg, sbuf, rbuf, own, fbuf, em, um, pbuf,
          in_sem, s1s, s1r, s2s, s2r, s3s, s3r, fs, fr):
    CAP, BASE, GRAN = cfg["cap"], cfg["base"], cfg["gran"]
    bits = []
    p = GRAN
    while p <= CAP - BASE:
        bits.append(p)
        p *= 2
    bits = bits[::-1]

    def scope(name):
        import contextlib
        return jax.named_scope(name) if cfg["scopes"] else contextlib.nullcontext()

    me = lax.axis_index("i")
    nbr = ((me + 1) & 3, (me + 3) & 3)

    ri_cp = pltpu.make_async_copy(ri_hbm, riv, in_sem.at[0])
    rw_cp = pltpu.make_async_copy(rw_hbm, rwv, in_sem.at[1])
    x_cp = [pltpu.make_async_copy(x_hbm.at[pl.ds(b * TB, TB)], xv.at[pl.ds(b * TB, TB)],
                                  in_sem.at[2 + b]) for b in range(NB)]

    def w_cp(c):
        col = c * CW if isinstance(c, int) else pl.multiple_of(c * CW, CW)
        return pltpu.make_async_copy(w_hbm.at[:, :, pl.ds(col, CW)], wv.at[c], in_sem.at[2 + NB + c])

    ri_cp.start()
    rw_cp.start()
    for cp in x_cp:
        cp.start(priority=cfg.get("prio", 0))
    for c in range(NC):
        w_cp(c).start(priority=cfg.get("prio", 0))

    barrier = pltpu.get_barrier_semaphore()
    for n in nbr:
        pl.semaphore_signal(barrier, inc=1, device_id=(n,), device_id_type=MESH)

    xg[pl.ds(0, 2 * CAP), :] = jnp.zeros((2 * CAP, D_IN), BF16)
    gg[:, pl.ds(0, 2 * CAP), :] = jnp.zeros((E_LOC, 2 * CAP, CW), F32)

    ri_cp.wait()
    with scope("plan"):
        e0 = riv[pl.ds(0, 8, stride=2), :] & (N_EXP - 1)
        e1 = riv[pl.ds(1, 8, stride=2), :] & (N_EXP - 1)
        c0, c1 = e0 >> 2, e1 >> 2
        diff = (c1 - c0) & 3
        is_s, is_d = diff == 0, diff == 2
        lead = jnp.where(diff == 3, c1, c0)
        cls = jnp.where(is_s, c0, jnp.where(is_d, 8 + (c0 & 1), 4 + lead))

        sub = _iota((8, 128), 0)
        odd = (sub & 1) == 1

        def per_block(pre, tot):
            prev = pltpu.roll(tot, 1, 0)
            nxt = pltpu.roll(tot, 7, 0)
            return pre + jnp.where(odd, prev, 0), tot + jnp.where(odd, prev, nxt)

        def after(tot, steps):
            for s in steps:
                tot = tot + jnp.where(sub >= s, pltpu.roll(tot, s, 0), 0)
            return tot

        pre, tot = _count([cls == k for k in range(10)])
        rank, cnt = zip(*[per_block(p_, t_) for p_, t_ in zip(pre, tot)])
        s, a, dg = cnt[:4], cnt[4:8], cnt[8:]
        d = [None] * 4
        d[1] = dg[0] >> 1
        d[3] = dg[0] - d[1]
        d[0] = (dg[1] * cfg["f0"]) >> 8
        d[2] = dg[1] - d[0]
        off = []
        for h in range(4):
            step = s[h] + a[h] + d[h] - HS
            off.append(step if h == 0 else off[-1] + step)
        lo = functools.reduce(jnp.maximum, [-o for o in off])
        hi = functools.reduce(jnp.minimum, [a[h] - off[h] for h in range(4)])
        mid = (a[0] + a[1] + a[2] + a[3] - 2 * (off[0] + off[1] + off[2] + off[3]) + 4) >> 3
        t = jnp.minimum(jnp.maximum(mid, lo), hi)
        up = [t + o for o in off]

        bad = lo > hi
        for m in range(4):
            for n in (up[m] + d[(m + 1) & 3], a[m] - up[m] + d[m]):
                end = after(n, (2, 4))
                bad |= end - jnp.minimum((end - n) & ~15, CAP - WIN) > WIN
        bad = jnp.where(bad, 1, 0)
        for sh in (4, 2):
            bad = bad | pltpu.roll(bad, sh, 0)

        my_rank = _pick(cls - 4, rank[4:])
        cut = _pick(cls - 4, up + [d[1], d[2]])
        first = my_rank < cut
        home = jnp.where(is_s, c0, jnp.where(
            is_d, (c0 & 1) + jnp.where(first, 1, 3), lead + jnp.where(first, 1, 0)))
        rel = (home - me) & 3

        def on(chip):
            return (c0 == chip) | (c1 == chip)

        lists = [on(me) & (rel == 1), on(me) & (rel == 3),
                 on(nbr[1]) & (rel == 0), on(nbr[0]) & (rel == 0)]
        pre, tot = _count([rel == h for h in range(4)] + lists)
        slot = _pick(rel, [per_block(pre[h], tot[h])[0] for h in range(4)])
        pos, start, length = [], [], []
        for k in range(4):
            end = after(tot[4 + k], (1, 2, 4))
            begin = end - tot[4 + k]
            w0 = jnp.minimum(jnp.where(odd, pltpu.roll(begin, 1, 0), begin) & ~15, CAP - WIN)
            pos.append(jnp.where(lists[k], begin + pre[4 + k] - w0, -1))
            start.append([0] + [pl.multiple_of(w0[2 * b, 0], 16) for b in range(1, NB)])
            length.append(end[7, 0])
        own_slot = jnp.where(rel == 0, slot, -1)
        fast = bad[0, 0] == 0

    rw_cp.wait()

    def gates(b, xb):
        scores = _dot_nt(rwv[...].astype(BF16), xb)
        probs = jnp.exp(scores - jnp.max(scores, axis=0, keepdims=True))
        probs = probs / jnp.sum(probs, axis=0, keepdims=True)
        b0, b1 = _block_lanes(e0, b), _block_lanes(e1, b)
        row = _iota((N_EXP, TB), 0)
        g0 = jnp.sum(jnp.where(row == b0, probs, 0.0), axis=0, keepdims=True)
        g1 = jnp.sum(jnp.where(row == b1, probs, 0.0), axis=0, keepdims=True)
        gs = g0 + g1
        mine = me * E_LOC + (_iota((8, TB), 0) & 3)
        return jnp.where(mine == b0, g0 / gs, 0.0) + jnp.where(mine == b1, g1 / gs, 0.0)

    def onehot(v, rows):
        return jnp.where(_iota((rows, TB), 0) == v, 1.0, 0.0).astype(BF16)

    def experts(c, lhs, gate):
        acc = None
        for e in range(E_LOC):
            y = gate(e) * _dot(lhs, wv[c, e].astype(BF16))
            acc = y if acc is None else acc + y
        return acc

    @pl.when(fast)
    def _():
        for b in range(NB):
            x_cp[b].wait()
            with scope("gather"):
                xb = xv[pl.ds(b * TB, TB), :].astype(BF16)
                sel = jnp.concatenate([onehot(_block_lanes(v, b), WIN)
                                       for v in (pos[0], pos[1], own_slot)], axis=0)
                rows = _dot(sel, xb)
                g = _dot_nt(sel, jnp.tile(gates(b, xb), (16, 1)).astype(BF16))
                for k in range(3):
                    at = k * CAP + (start[k][b] if k < 2 else b * HS)
                    r = rows[k * WIN:(k + 1) * WIN]
                    merge = k < 2 and b > 0
                    if merge:
                        r = r + xg[pl.ds(at, WIN), :].astype(F32)
                    xg[pl.ds(at, WIN), :] = r.astype(BF16)
                    for e in range(E_LOC):
                        ge = jnp.broadcast_to(g[k * WIN:(k + 1) * WIN, e:e + 1], (WIN, CW))
                        if merge:
                            ge = ge + gg[e, pl.ds(at, WIN), :]
                        gg[e, pl.ds(at, WIN), :] = ge

        def pieces(k, c, action):
            j = k & 1
            extra = jnp.maximum(length[k] - BASE + (GRAN - 1), 0)

            def piece(i, at, rows):
                action(pltpu.make_async_remote_copy(
                    sbuf.at[c, pl.ds(j * CAP + at, rows)], rbuf.at[c, pl.ds(j * CAP + at, rows)],
                    s1s.at[c, j, i], s1r.at[c, j, i], device_id=(nbr[j],), device_id_type=MESH))

            piece(0, 0, BASE)
            for i, bit in enumerate(bits):
                at = pl.multiple_of(BASE + (extra & ~(2 * bit - 1)), 2 * GRAN)
                pl.when((extra & bit) != 0)(functools.partial(piece, i + 1, at, bit))

        def half(c, h, j):
            return fbuf.at[c, h, pl.ds(j * 2 * HS, 2 * HS)]

        def bcast(c, j, part):
            return pltpu.make_async_remote_copy(
                half(c, 0, j ^ part), half(c, 3 - 2 * j, j ^ part), s2s.at[c, j, part],
                s2r.at[c, j, part], device_id=(nbr[j],), device_id_type=MESH)

        def relay(c, j):
            return pltpu.make_async_remote_copy(
                half(c, 3 - 2 * j, j), half(c, 2, j), s3s.at[c, j], s3r.at[c, j],
                device_id=(nbr[j],), device_id_type=MESH)

        def stage1(c):
            w_cp(c).wait()
            with scope("mm_send"):
                z = experts(c, xg[pl.ds(0, 2 * CAP), :], lambda e: gg[e, pl.ds(0, 2 * CAP), :])
                sbuf[c] = z.astype(BF16)
            for k in range(2):
                pieces(k, c, lambda cp: cp.start())

        def local(c):
            with scope("mm_own"):
                own[c] = experts(c, xg[pl.ds(2 * CAP, NB * HS), :],
                                 lambda e: gg[e, pl.ds(2 * CAP, NB * HS), :])

        def reduce(c):
            with scope("wait1"):
                for k in (2, 3):
                    pieces(k, c, lambda cp: cp.wait_recv())
            with scope("reduce"):
                for b in range(NB):
                    got = []
                    for k in (2, 3):
                        v = rbuf[c, pl.ds((k & 1) * CAP + start[k][b], WIN), :].astype(F32)
                        ok = _iota((WIN, CW), 0) < length[k] - start[k][b]
                        got.append(jnp.where(ok, v, 0.0).astype(BF16))
                    rows = pl.ds(b * HS, HS)
                    f = own[c, rows, :] + _dot(em[rows, :], jnp.concatenate(got, axis=0))
                    fbuf[c, 0, rows, :] = f.astype(BF16)

        def stage2(c, part):
            for j in range(2):
                bcast(c, j, part).start()

        def stage3(c):
            with scope("wait2a"):
                for j in range(2):
                    bcast(c, j, 0).wait_recv()
                    relay(c, j).start()

        def finish(c):
            col = c * CW if isinstance(c, int) else pl.multiple_of(c * CW, CW)
            with scope("wait3"):
                for j in range(2):
                    bcast(c, j, 1).wait_recv()
                    relay(c, j).wait_recv()
            with scope("unperm"):
                for b in range(NB):
                    rhs = jnp.concatenate([fbuf[c, h, pl.ds(b * HS, HS), :] for h in range(4)], axis=0)
                    out_ref[pl.ds(b * TB, TB), pl.ds(col, CW)] = _dot(
                        um[pl.ds(b * TB, TB), :], rhs).astype(out_ref.dtype)

        def drain(c):
            for k in range(2):
                pieces(k, c, lambda cp: cp.wait_send())
            for j in range(2):
                bcast(c, j, 0).wait_send()
                bcast(c, j, 1).wait_send()
                relay(c, j).wait_send()

        def tables():
            with scope("tables"):
                for b in range(NB):
                    src = jnp.concatenate([onehot(_block_lanes(pos[k], b), WIN) for k in (2, 3)], axis=0)
                    em[pl.ds(b * HS, HS), :] = _dot_nt(
                        onehot(_block_lanes(own_slot, b), HS), src).astype(BF16)
                where = rel * HS + slot
                for r in range(8):
                    col = jnp.broadcast_to(where[r:r + 1], (128, 128)).T
                    for i in range(2):
                        um[pl.ds(r * 128, 128), pl.ds(i * 128, 128)] = jnp.where(
                            col == _iota((128, 128), 1) + i * 128, 1.0, 0.0).astype(BF16)

        pl.semaphore_wait(barrier, 2)
        stage1(0)
        tables()
        local(0)
        if cfg["loop"]:
            def step(i, carry):
                pl.when(i < NC)(lambda: stage1(i))

                @pl.when(i < NC + 1)
                def _():
                    reduce(i - 1)
                    stage2(i - 1, 0)
                    stage2(i - 1, 1)
                pl.when((i >= 2) & (i < NC + 2))(lambda: stage3(i - 2))
                pl.when(i < NC)(lambda: local(i))

                @pl.when(i >= 3)
                def _():
                    drain(i - 3)
                    finish(i - 3)
                return carry
            lax.fori_loop(1, NC + 3, step, 0)
        else:
            for i in range(1, NC + 3):
                if i < NC:
                    stage1(i)
                if i < NC + 1:
                    reduce(i - 1)
                    stage2(i - 1, 0)
                    stage2(i - 1, 1)
                if 2 <= i < NC + 2:
                    stage3(i - 2)
                if i < NC:
                    local(i)
                if i >= 3:
                    drain(i - 3)
                    finish(i - 3)

    @pl.when(jnp.logical_not(fast))
    def _():
        for b in range(NB):
            x_cp[b].wait()
            g = gates(b, xv[pl.ds(b * TB, TB), :].astype(BF16))
            for i in range(2):
                for e in range(E_LOC):
                    gg[e, pl.ds(b * TB + i * 128, 128), :] = jnp.broadcast_to(
                        g[e:e + 1, i * 128:(i + 1) * 128], (128, 128)).T
        pl.semaphore_wait(barrier, 2)

        def chunk(c, carry):
            w_cp(c).wait()

            def block(b, carry):
                rows = pl.ds(pl.multiple_of(b * TB, TB), TB)
                pbuf[c, 0, rows, :] = experts(
                    c, xv[rows, :].astype(BF16), lambda e: gg[e, rows, :]).astype(BF16)
                return carry
            lax.fori_loop(0, NB, block, 0)
            for i, peer in enumerate((me ^ 1, 3 - me)):
                cp = pltpu.make_async_remote_copy(
                    pbuf.at[c, 2 * i], pbuf.at[c, 2 * i + 1], fs.at[c, i], fr.at[c, i],
                    device_id=(peer,), device_id_type=MESH)
                cp.start()
                cp.wait()
                total = pbuf[c, 2 * i].astype(F32) + pbuf[c, 2 * i + 1].astype(F32)
                if i == 0:
                    pbuf[c, 2] = total.astype(BF16)
                else:
                    out_ref[:, pl.ds(pl.multiple_of(c * CW, CW), CW)] = total.astype(out_ref.dtype)
            return carry
        lax.fori_loop(0, NC, chunk, 0)


def make(**kw):
    cfg = dict(DEFAULT, **kw)
    cap = cfg["cap"]

    def kernel(x, router_W, route_idx, expert_W):
        dma = pltpu.SemaphoreType.DMA
        ri = route_idx.astype(I32).reshape(8, 128, 2).transpose(0, 2, 1).reshape(16, 128)
        return pl.pallas_call(
            functools.partial(_body, cfg),
            out_shape=jax.ShapeDtypeStruct((N_TOK, D_OUT), cfg.get("out_dtype", BF16)),
            in_specs=[pl.BlockSpec(memory_space=pl.ANY)] * 4,
            out_specs=pl.BlockSpec(memory_space=pltpu.VMEM),
            scratch_shapes=[
                pltpu.VMEM((N_TOK, D_IN), F32),
                pltpu.VMEM((N_EXP, D_IN), F32),
                pltpu.VMEM((16, 128), I32),
                pltpu.VMEM((NC, E_LOC, D_IN, CW), F32),
                pltpu.VMEM((2 * cap + NB * HS, D_IN), BF16),
                pltpu.VMEM((E_LOC, N_TOK, CW), F32),
                pltpu.VMEM((NC, 2 * cap, CW), BF16),
                pltpu.VMEM((NC, 2 * cap, CW), BF16),
                pltpu.VMEM((NC, NB * HS, CW), F32),
                pltpu.VMEM((NC, N_DEV, NB * HS, CW), BF16),
                pltpu.VMEM((NB * HS, 2 * WIN), BF16),
                pltpu.VMEM((N_TOK, TB), BF16),
                pltpu.VMEM((NC, 4, N_TOK, CW), BF16),
                dma((2 + NB + NC,)),
                dma((NC, 2, 7)), dma((NC, 2, 7)),
                dma((NC, 2, 2)), dma((NC, 2, 2)),
                dma((NC, 2)), dma((NC, 2)),
                dma((NC, 2)), dma((NC, 2)),
            ],
            compiler_params=pltpu.CompilerParams(
                collective_id=0, vmem_limit_bytes=48 * 2**20,
                disable_semaphore_checks=cfg.get("nosem", True),
                disable_bounds_checks=cfg.get("nobounds", True)),
        )(x, router_W.T, ri, expert_W)
    return kernel


def pallas_dist_moe_top2_ep_n1024_d512_e4_h1024_kernel(x, router_W, route_idx, expert_W):
    return make()(x, router_W, route_idx, expert_W)
```

```python
import contextlib
import functools

import jax
import jax.numpy as jnp
from jax import lax
from jax.experimental import pallas as pl
from jax.experimental.pallas import tpu as pltpu

N_TOK, D_IN, D_OUT = 1024, 512, 1024
N_DEV, E_LOC, N_EXP = 4, 4, 16
NB, TB, HS = 4, 256, 64
NG, GS = 2, 128
NC, CW = 8, 128
EW = 64
YR = E_LOC * EW
BF16, F32, I32 = jnp.bfloat16, jnp.float32, jnp.int32
MESH = pl.DeviceIdType.MESH

HEAD = ("X x0 I0 X X i0 I1 U i1 x1 B V0 w0 P0 s0a w1 P1 s0b i2 z0 I2 y i3 z1 I3 s1 W2 W3 W4 W5 W6 W7 "
        "w2 q0a P2 O0a A0a a0a w3 q0b P3 O0b A0b a0b o1 r1a A1a a1a r1b A1b a1b")
REST = ("| [Vs,R,qOA,a,F,H,t] Vs2 R0 Vs3 R1 Vs4 qOA2 a2 Vs5 qOA3 a3 Vs6 qOA4 a4 Vs7 qOA5 a5 F2 H0 t0 F3 "
        "qOA6 F4 H1 t1 qOA7 | R5 a6 | [R,L,G,t] G2 t2 R6 G3 t3 L7 G4 t4 | g H+5 t+5 | l7")
DEFAULT = dict(cap=112, whole=(96, 64, 32, 16, 8, 4, 2), part=((56, 32, 16, 8), (52, 32, 16, 8, 4)), delta=24, bias=24, gs=6, scopes=False, head=HEAD, rest=REST,
               fix=(112, 104), soft=(136, 136, 120, 136), fx=32, nf=4, prio=1, first=2, ne=3)


def _dot(a, b):
    return jnp.dot(a, b, preferred_element_type=F32)


def _dot_nt(a, b):
    return lax.dot_general(a, b, (((1,), (1,)), ((), ())), preferred_element_type=F32)


def _wide(ref, *idx):
    return jnp.concatenate([ref[(j, *idx)] for j in range(ref.shape[0])], axis=1)


def _put(ref, rows, value):
    for j in range(ref.shape[0]):
        ref[j, rows, :] = value[:, j * 128:(j + 1) * 128].astype(ref.dtype)


def _apply(ref, first, n, rhs):
    half = (n + 16) // 32 * 16
    return jnp.concatenate([_dot(_wide(ref, pl.ds(first + r, m)), rhs)
                            for r, m in ((0, half), (half, n - half))], axis=0)


def _iota(shape, dim):
    return lax.broadcasted_iota(I32, shape, dim)


def _ones(mask):
    return jnp.where(mask, 1.0, 0.0)


def _count(flags):
    tri = _ones(_iota((128, 256), 0) < _iota((128, 256), 1)).astype(BF16)
    r = _dot(jnp.concatenate(flags, axis=0).astype(BF16), tri).astype(I32)
    return [(r[8 * k:8 * k + 8, :128], r[8 * k:8 * k + 8, 128:]) for k in range(len(flags))]


def _pick(idx, vals):
    out = vals[-1]
    for k in range(len(vals) - 2, -1, -1):
        out = jnp.where(idx == k, vals[k], out)
    return out


def _choose(idx, vals):
    return vals[idx] if isinstance(idx, int) else _pick(idx, vals)


def _aligned(i, n):
    return i if isinstance(i, int) else pl.multiple_of(i, n)


def _lanes(v, first=0, n=8):
    return jnp.concatenate([v[r:r + 1] for r in range(first, first + n)], axis=1)


def _scatter(*parts):
    pos = jnp.concatenate([_lanes(p) for p, _ in parts], axis=1)
    n = pos.shape[1]
    hit = (pos >> 7) == _iota((8, n), 0)
    lhs = [jnp.where(hit, jnp.concatenate([_lanes(v) for v in vals], axis=1), 0).astype(F32)
           for vals in zip(*[v for _, v in parts])]
    if len(lhs) % 2:
        lhs.append(jnp.zeros((8, n), F32))
    out = _dot_nt(jnp.concatenate(lhs, axis=0).astype(BF16),
                  _ones((pos & 127) == _iota((128, n), 0)).astype(BF16)).astype(I32)
    return [out[8 * k:8 * k + 8] for k in range(len(parts[0][1]))]


def _body(cfg, x_hbm, rw_hbm, ri_hbm, w_hbm, out_ref,
          rwv, riv, iv, ism0, ism1, tab, wv, xs0, xs1, xs2, xs3, xg, cs, co, em, um, sbuf, rbuf, own, fbuf,
          xv, xd, gg, pbuf, wsem, isem, xsem, ssem, r1, r2, r3):
    CAP, FX, NF = cfg["cap"], cfg["fx"], cfg["nf"]
    xs = ((xs0, xs1), (xs2, xs3))
    ism = (ism0, ism1)

    def scope(name):
        on_ = cfg["scopes"] is True or (cfg["scopes"] and name[0] in cfg["scopes"])
        return jax.named_scope(name) if on_ else contextlib.nullcontext()

    me = lax.axis_index("i")
    nbr = ((me + 1) & 3, (me + 3) & 3)

    def col_of(c):
        return pl.ds(_aligned(c * CW, CW), CW)

    ri_cp = pltpu.make_async_copy(ri_hbm, riv, wsem.at[NC])
    rw_cp = pltpu.make_async_copy(rw_hbm, rwv, wsem.at[NC + 1])

    def idx_cp(i):
        return pltpu.make_async_copy(iv.at[i], ism[i], isem.at[i])

    def w_cp(c):
        return pltpu.make_async_copy(w_hbm.at[:, :, col_of(c)], wv.at[c], wsem.at[c])

    def w_part(i):
        es = (pl.ds(0, cfg["ne"]), pl.ds(cfg["ne"], E_LOC - cfg["ne"]))[i]
        return pltpu.make_async_copy(w_hbm.at[es, :, col_of(1)], wv.at[1, es], wsem.at[(1, NC + 2)[i]])

    ri_cp.start()
    rw_cp.start()
    for cp in (w_cp(0), w_part(0), w_part(1)):
        cp.start(priority=cfg["prio"])

    barrier = pltpu.get_barrier_semaphore()
    for n in nbr:
        pl.semaphore_signal(barrier, inc=1, device_id=(n,), device_id_type=MESH)

    for k in range(4):
        fix = cfg["fix"][k // 2]
        xs[k // 2][k % 2][:, pl.ds(fix, YR - fix), :] = jnp.zeros((4, YR - fix, 128), F32)

    ri_cp.wait()
    with scope("plan"):
        e0 = riv[pl.ds(0, 8, stride=2), :] & (N_EXP - 1)
        e1 = riv[pl.ds(1, 8, stride=2), :] & (N_EXP - 1)
        c0, c1 = e0 >> 2, e1 >> 2
        diff = (c1 - c0) & 3
        is_s, is_d = diff == 0, diff == 2
        lead = jnp.where(diff == 3, c1, c0)
        cls = jnp.where(is_s, c0, jnp.where(is_d, 8 + (c0 & 1), 4 + lead))
        sub = _iota((8, 128), 0)

        def widen(pre, tot, step):
            second = (sub & step) != 0
            prev, nxt = pltpu.roll(tot, step, 0), pltpu.roll(tot, 8 - step, 0)
            return pre + jnp.where(second, prev, 0), tot + jnp.where(second, prev, nxt)

        rank, cnt = zip(*[widen(*pt, 1) for pt in _count([_ones(cls == k) for k in range(10)])])
        s, a, dg = cnt[:4], cnt[4:8], cnt[8:]
        parity = (sub >> 1) & 1
        d1 = jnp.clip((dg[0] + s[1] - s[3] + parity) >> 1, 0, dg[0])
        q0 = s[0] + a[0] - HS
        q1 = q0 + s[1] + a[1] + d1 - HS
        q2 = q1 + s[2] + a[2] + dg[1] - HS
        d0 = (dg[1] + s[0] - s[2] + parity - cfg["delta"]) >> 1
        d0 = jnp.maximum(d0, jnp.maximum(q2 - a[2], -a[3]) - jnp.minimum(q0, q1))
        d0 = jnp.minimum(d0, jnp.minimum(a[0] - q0, a[1] - q1) + jnp.minimum(q2, 0))
        d0 = jnp.clip(d0, 0, dg[1])
        d = [d0, d1, dg[1] - d0, dg[0] - d1]
        off = [q0 + d0, q1 + d0, q2, jnp.zeros_like(q2)]
        lo = functools.reduce(jnp.maximum, [-o for o in off])
        hi = functools.reduce(jnp.minimum, [a[h] - off[h] for h in range(4)])
        mid = (a[0] + a[1] + a[2] + a[3] - 2 * (off[0] + off[1] + off[2]) + 4) >> 3
        t = jnp.minimum(jnp.maximum(mid, lo), hi)
        up = [t + o for o in off]

        first = _pick(cls - 4, rank[4:]) < _pick(cls - 4, up + [d[1], d[2]])
        home = jnp.where(is_s, c0, jnp.where(
            is_d, (c0 & 1) + jnp.where(first, 1, 3), lead + jnp.where(first, 1, 0)))
        rel = (home - me) & 3

        def on(chip):
            return (c0 == chip) | (c1 == chip)

        def layout(counts):
            begin = [jnp.zeros((8, 128), I32)]
            for _, tot in counts:
                begin.append(begin[-1] + tot)
            return begin

        sent = on(me) & (rel != 0)
        mine = jnp.where(c0 == me, e0, e1) & 3
        by_e = [widen(*widen(*pt, 1), 2)
                for pt in _count([_ones(sent & (mine == e)) for e in range(E_LOC)])]
        send_first = layout(by_e)
        token = sub * 128 + _iota((8, 128), 1)
        base = (sub >> 2) * YR
        send_rank = _pick(mine, [pre for pre, _ in by_e])
        got = _scatter((jnp.where(sent, base + _pick(mine, send_first[:4]) + send_rank, -1),
                        (token >> 3, token & 7)))
        iv[0] = (got[0] * 8 + got[1]) & (N_TOK - 1)
        idx_cp(0).start()

        cw = [widen(0, up[m] + d[(m + 1) & 3], 2)[1] for m in range(4)]
        ccw = [widen(0, a[m] - up[m] + d[m], 2)[1] for m in range(4)]
        bad = (lo > hi) | (functools.reduce(jnp.maximum, cw + ccw) > CAP - 2)
        bad = jnp.where(bad, 1, 0)
        bins = _iota((2 * N_EXP, N_TOK), 0)
        load = (_ones(_lanes(e0 + jnp.where(c0 == home, N_EXP, 0)) == bins)
                + _ones(_lanes(e1 + jnp.where(c1 == home, N_EXP, 0)) == bins))
        for g in range(NG):
            over = jnp.sum(load[:, g * 2 * TB:(g + 1) * 2 * TB], axis=1, keepdims=True) > EW
            for i in range(4):
                bad = bad | jnp.where(over[8 * i:8 * i + 8], 1, 0)
        for sh in (4, 2, 1):
            bad = bad | pltpu.roll(bad, sh, 0)
        lean = []
        for m in range(4):
            gap = ccw[m] - cw[(m - 1) & 3]
            lean.append(((((gap + pltpu.roll(gap, 4, 0)) * cfg["gs"]) >> 3) + cfg["bias"] * (0, 1, 0, -1)[m] + FX // 8)
                        >> ((FX // 4).bit_length() - 1))
        lean = [_pick(n + 0 * sub, lean)[0, 0] for n in nbr]
        fast = bad[0, 0] == 0
    rw_cp.wait()

    def picked(xb, b0, b1):
        scores = _dot_nt(rwv[...].astype(BF16), xb)
        probs = jnp.exp(scores - jnp.max(scores, axis=0, keepdims=True))
        probs = probs / jnp.sum(probs, axis=0, keepdims=True)
        expert = _iota(scores.shape, 0)
        return (jnp.sum(jnp.where(expert == b0, probs, 0.0), axis=0, keepdims=True),
                jnp.sum(jnp.where(expert == b1, probs, 0.0), axis=0, keepdims=True))

    @pl.when(jnp.logical_not(fast))
    def _():
        x_cp = pltpu.make_async_copy(x_hbm, xv, isem.at[1])
        x_cp.start()
        for c in range(cfg["first"], NC):
            w_cp(c).start(priority=cfg["prio"])
        x_cp.wait()
        idx_cp(0).wait()

        def prepare(r, carry):
            rows = pl.ds(pl.multiple_of(r * 128, 128), 128)
            xb = jnp.concatenate([xv[pl.ds(r * 16, 16), j].reshape(128, 128) for j in range(4)],
                                 axis=1).astype(BF16)
            xd[rows, :] = xb
            b0, b1 = (riv[pl.ds(2 * r + k, 1), :] & (N_EXP - 1) for k in range(2))
            g0, g1 = picked(xb, b0, b1)
            for e in range(E_LOC):
                g = (jnp.where(b0 == me * E_LOC + e, g0 / (g0 + g1), 0.0)
                     + jnp.where(b1 == me * E_LOC + e, g1 / (g0 + g1), 0.0))
                gg[e, rows, :] = jnp.broadcast_to(g, (128, 128)).T
            return carry
        lax.fori_loop(0, 8, prepare, 0)
        pl.semaphore_wait(barrier, 2)

        w_part(0).wait()
        w_part(1).wait()

        def chunk(c, carry):
            pl.when(c != 1)(lambda: w_cp(c).wait())

            def block(b, carry):
                rows = pl.ds(pl.multiple_of(b * 128, 128), 128)
                pbuf[c, 0, rows, :] = sum(
                    gg[e, rows, :] * _dot(xd[rows, :], wv[c, e].astype(BF16))
                    for e in range(E_LOC)).astype(BF16)
                return carry
            lax.fori_loop(0, 8, block, 0)
            for i, peer in enumerate((me ^ 1, 3 - me)):
                cp = pltpu.make_async_remote_copy(
                    pbuf.at[c, 2 * i], pbuf.at[c, 2 * i + 1], ssem.at[c], r3.at[c, i],
                    device_id=(peer,), device_id_type=MESH)
                cp.start()
                cp.wait()
                total = pbuf[c, 2 * i].astype(F32) + pbuf[c, 2 * i + 1].astype(F32)
                if i == 0:
                    pbuf[c, 2] = total.astype(BF16)
                else:
                    out_ref[:, col_of(c)] = total.astype(out_ref.dtype)
            return carry
        lax.fori_loop(0, NC, chunk, 0)

    @pl.when(fast)
    def _():
        length = []
        edge = [[[0, 0]] + [[v[4 * g, 0] for g in range(NG)] for v in send_first[1:]]]

        def tables():
            kept = [(c0 == me) & (rel == 0), (c1 == me) & (rel == 0)]
            lists = [sent & (rel == 1), sent & (rel == 3),
                     on(nbr[1]) & (rel == 0), on(nbr[0]) & (rel == 0)]
            flags = [_ones(rel == h) for h in range(4)] + [_ones(f) for f in lists]
            flags += [_ones(kept[0] & ((e0 & 3) == e)) + _ones(kept[1] & ((e1 & 3) == e))
                      for e in range(E_LOC)]
            counts = [widen(*pt, 1) for pt in _count(flags)]
            slot = _pick(rel, [counts[h][0] for h in range(4)])
            counts = [widen(*pt, 2) for pt in counts[4:]]
            row = [jnp.where(sub < 4, CAP - 1 - counts[k][0], counts[k][0]) for k in range(4)]
            length.extend([[counts[k][1][4 * g, 0] for g in range(NG)] for k in range(4)])
            own_first = layout(counts[4:])
            edge.append([[0, 0]] + [[v[4 * g, 0] for g in range(NG)] for v in own_first[1:]])
            pre = [p for p, _ in counts[4:]]
            own_rank = [_pick(e0 & 3, pre), _pick(e1 & 3, pre) + jnp.where(e0 == e1, 1, 0)]
            got = _scatter(*[
                (jnp.where(kept[k], base + _pick(e & 3, own_first[:4]) + own_rank[k], -1),
                 (token >> 3, token & 7)) for k, e in enumerate((e0, e1))])
            iv[1] = (got[0] * 8 + got[1]) & (N_TOK - 1)
            idx_cp(1).start()
            yield
            my_slot = (sub & 2) * (HS // 2) + slot + 1
            target = jnp.where(rel == 0, my_slot, jnp.where(rel == 1, row[0], CAP + row[1]) + 1)
            tab[0], tab[1] = _scatter(*[
                (jnp.where(c == me, base + (e & 3) * EW
                           + jnp.where(rel == 0, NG * YR + own_rank[k], send_rank), -1), (target, other))
                for k, (c, e, other) in enumerate(((c0, e0, e1), (c1, e1, e0)))])
            yield
            (came,) = _scatter(*[(jnp.where(lists[k], base + (k - 2) * 128 + row[k], -1), (my_slot,)) for k in (2, 3)])
            for g in range(NG):
                _put(em, pl.ds(g * GS, GS),
                     _ones(_lanes(came, 2 * g, 2) == _iota((GS, YR), 0) + 1))
            yield
            (who,) = _scatter(((sub >> 1) * TB + rel * HS + slot, (token & (TB - 1),)))
            for b in range(NB):
                _put(um, pl.ds(b * TB, TB),
                     _ones(_lanes(who, 2 * b, 2) == _iota((TB, TB), 0)))
            yield

        table_steps = tables()

        def fetch(k, g, first, n, run):
            p = g * YR + first
            for i in range(n):
                tok = ism[k][p >> 7, (p & 127) + i]
                pltpu.make_async_copy(x_hbm.at[tok >> 3, :, pl.ds(tok & 7, 1), :],
                                      xs[k][g].at[:, pl.ds(first + i, 1), :], xsem.at[k, g, run]).start()

        def fetched(k, g, first, n, run):
            dst = xs[k][g].at[:, pl.ds(_aligned(first, 8), n), :]
            pltpu.make_async_copy(dst, dst, xsem.at[k, g, run]).wait()

        def likely(k, g, action):
            fix = cfg["fix"][k]
            action(k, g, 0, fix, 0)
            for i in range((cfg["soft"][2 * k + g] - fix) // 8):
                pl.when(fix + 8 * i < edge[k][E_LOC][g])(
                    functools.partial(action, k, g, fix + 8 * i, 8, i + 1))

        def more(k, g, action):
            fix = cfg["fix"][k]
            done = (cfg["soft"][2 * k + g] - fix) // 8
            runs = jnp.maximum((edge[k][E_LOC][g] - fix + 7) >> 3, done)
            lax.fori_loop(done, runs, lambda i, _: action(k, g, fix + 8 * i, 8, i + 1), None)

        def prepare(k, g):
            xb = []
            for e in range(E_LOC):
                rows = pl.ds((k * NG + g) * EW, EW)
                _put(xg.at[e], rows, _wide(xs[k][g], pl.ds(edge[k][e][g], EW)))
                xb.append(_wide(xg.at[e], rows))
            target, other = (jnp.concatenate([tab[i, pl.ds(2 * (k * NG + g) + r, 1), :] for r in range(2)],
                                             axis=1) for i in range(2))
            g0, g1 = picked(jnp.concatenate(xb, axis=0), me * E_LOC + _iota((1, YR), 1) // EW, other)
            ref, n = ((cs, 2 * CAP), (co, GS))[k]
            _put(ref, pl.ds(_aligned(g * n, 16), n),
                 jnp.where(target == _iota((n, YR), 0) + 1, g0 / (g0 + g1), 0.0))

        def remote(src, dst, c, recv_sem, j):
            return pltpu.make_async_remote_copy(
                src, dst, ssem.at[c], recv_sem, device_id=(_choose(j, nbr),), device_id_type=MESH)

        def pieces(ks, c, gs, action):
            if isinstance(c, int) and c < 2 and len(gs) == NG:
                for g in gs:
                    pieces(ks, c, (g,), action)
                return
            sizes = cfg["whole"] if len(gs) == NG else cfg["part"][c]
            unit = sizes[-1]
            at, stop = [], []
            for k in ks:
                at.append((CAP - length[k][0]) & -unit if 0 in gs else CAP)
                stop.append(CAP + length[k][1] if 1 in gs else CAP)
                if gs == (0,):
                    at[-1] = jnp.minimum(at[-1], CAP - sizes[0])

            def piece(j, i, first, n):
                rows = pl.ds(_aligned(first, unit), n)
                action(remote(sbuf.at[c, j, rows], rbuf.at[c, j, rows], c,
                              r1.at[c, j, gs[0] * len(sizes) + i], j))

            for i, n in enumerate(sizes):
                for j in range(2):
                    if i == 0:
                        piece(j, i, at[j], n)
                        at[j] = at[j] + n
                    else:
                        fits = at[j] + n < stop[j] + unit
                        pl.when(fits)(functools.partial(piece, j, i, at[j], n))
                        at[j] = at[j] + jnp.where(fits, n, 0)

        def bcast(c, j, b, n=2):
            rows = pl.ds(_aligned(b * HS, HS), n * HS)
            return remote(fbuf.at[c, 0, rows], fbuf.at[c, 3 - 2 * j, rows], c, r2.at[c, j, (b + 2 * j + 2) & 3], j)

        def relay(c, j, i, n):
            rows = pl.ds(i * FX, n * FX)
            return remote(fbuf.at[c, 3 - 2 * j, rows], fbuf.at[c, 2, rows], c, r3.at[c, i], j)

        def relays(c, action):
            half = TB // FX // 2
            for i in range(2 * half):
                for j in range(2):
                    split = half + jnp.where(lean[j] > 0, jnp.maximum(lean[j] - (NF - c) * half, 0),
                                             jnp.minimum(lean[j] + (NF - c) * half, 0))
                    pl.when(i < split if j == 0 else i >= split)(
                        lambda i=i, j=j: action(relay(c, j, i, 1)))

        def leaf(c, j, b, n):
            return relay(c, j, b * HS // FX, n * HS // FX) if b // 2 == j else bcast(c, j, b, n)

        def arrived(c, g):
            r = _iota((CAP, CW), 0)
            got = []
            for j in range(2):
                used = r >= CAP - length[2 + j][0] if g == 0 else r < length[2 + j][1]
                got += [jnp.where(used, rbuf[c, j, pl.ds(g * CAP, CAP), :].astype(F32), 0.0),
                        jnp.zeros((128 - CAP, CW), F32)]
            return _apply(em, g * GS, GS, jnp.concatenate(got, axis=0).astype(BF16))

        early = []

        def expert(c, e, k, gs):
            rows = pl.ds((k * NG + gs[0]) * EW, len(gs) * EW)
            return _dot(_wide(xg.at[e], rows), wv[c, e].astype(BF16)).astype(BF16)

        def experts(c, k, gs, finish=False):
            y = early[:]
            del early[:]
            y += [expert(c, e, k, gs) for e in range(len(y), E_LOC)]
            for i, g in enumerate(gs):
                yk = jnp.concatenate([v[i * EW:(i + 1) * EW] for v in y], axis=0)
                if k == 0:
                    for j in range(2):
                        sbuf[c, j, pl.ds(g * CAP, CAP), :] = _dot(
                            _wide(cs, pl.ds((2 * g + j) * CAP, CAP)), yk).astype(BF16)
                elif finish:
                    fbuf[c, 0, pl.ds(g * GS, GS), :] = (
                        arrived(c, g) + _apply(co, g * GS, GS, yk)).astype(BF16)
                else:
                    own[pl.ds(g * GS, GS), :] = _apply(co, g * GS, GS, yk)
            if k == 0:
                pieces((0, 1), c, gs, lambda cp: cp.start())

        def unpermute(c, b):
            rhs = jnp.concatenate([fbuf[c, h, pl.ds(b * HS, HS), :] for h in range(4)], axis=0)
            out_ref[pl.ds(b * TB, TB), col_of(c)] = _apply(um, b * TB, TB, rhs).astype(out_ref.dtype)

        def drain(c):
            pl.when(c > 1)(lambda: pieces((0, 1), c, (0, 1), lambda cp: cp.wait_send()))
            for early in range(2):
                pl.when(c == early)(functools.partial(
                    pieces, (0, 1), early, (0, 1), lambda cp: cp.wait_send()))
            for j in range(2):
                bcast(c, j, 2 * j).wait_send()

        def run(op, i=0):
            kind, arg = op[0], op[1:]
            gs = (0, 1)
            if arg[-1:] in ("a", "b", "g"):
                gs, arg, i = (i if arg[-1] == "g" else "ab".index(arg[-1]),), arg[:-1], 0
            c = (i + int(arg)) if arg else None
            with scope(op):
                if kind in "IiwP":
                    k, g = int(arg) // 2, (i if arg[0] == "+" else int(arg) % 2)
                    if kind == "I":
                        likely(k, g, fetch)
                    elif kind == "i":
                        more(k, g, fetch)
                    elif kind == "w":
                        more(k, g, fetched)
                        likely(k, g, fetched)
                    else:
                        prepare(k, g)
                elif kind == "W":
                    w_cp(c).start(priority=cfg["prio"])
                elif kind == "V":
                    w_cp(c).wait()
                elif kind == "z":
                    w_part(c).wait()
                elif kind == "y":
                    early.extend(expert(1, e, 0, (0, 1)) for e in range(cfg["ne"]))
                elif kind == "B":
                    pl.semaphore_wait(barrier, 2)
                elif kind in "XU":
                    next(table_steps)
                elif kind == "x":
                    idx_cp(c).wait()
                elif kind in "soO":
                    experts(c, int(kind != "s"), gs, kind == "O")
                elif kind in "qr":
                    pieces((2, 3), c, gs, lambda cp: cp.wait_recv())
                    for g in gs if kind == "r" else ():
                        rows = pl.ds(_aligned(g * GS, GS), GS)
                        fbuf[c, 0, rows, :] = (own[rows, :] + arrived(c, g)).astype(BF16)
                elif kind == "A":
                    for g in gs:
                        bcast(c, g, 2 * g).start()
                elif kind == "a":
                    for g in gs:
                        bcast(c, 1 - g, 2 * g).start()
                elif kind == "F":
                    for j in range(2):
                        for b in (0, 2):
                            bcast(c, j, b).wait_recv()
                    relays(c, lambda cp: cp.start())
                elif kind == "R":
                    for g in gs:
                        bcast(c, g, 2 * g).wait_recv()
                        leaf(c, g, 2 * g, 2).start()
                elif kind == "L":
                    for j in range(2):
                        bcast(c, j, 2 * j).wait_recv()
                    for b in range(NB):
                        for j in range(2):
                            leaf(c, j, b, 1).start()
                elif kind == "G":
                    for j in range(2):
                        bcast(c, j, 2 - 2 * j).wait_send()
                    relays(c, lambda cp: cp.wait_send())
                    for i in range(TB // FX):
                        relay(c, 0, i, 1).wait_recv()
                elif kind == "H":
                    for b in (0, 2):
                        for j in range(2):
                            leaf(c, j, b, 2).wait_send()
                            leaf(c, j, b, 2).wait_recv()
                elif kind == "t":
                    drain(c)
                    for b in range(NB):
                        unpermute(c, b)
                elif kind == "l":
                    drain(c)
                    for b in range(NB):
                        for j in range(2):
                            with scope("l-recv"):
                                leaf(c, j, b, 1).wait_recv()
                        unpermute(c, b)
                    for j in range(2):
                        with scope("l-send"):
                            for b in range(NB):
                                leaf(c, j, b, 1).wait_send()
                else:
                    raise ValueError(op)

        for part in (cfg["head"] + " " + cfg["rest"]).split("|"):
            ops = part.split()
            if ops and ops[0] == "g":
                def step(i, carry, ops=ops):
                    for op in ops[1:]:
                        run(op, i)
                    return carry
                lax.fori_loop(0, NG, step, 0)
            elif ops and ops[0][0] == "[":
                body = ops[0][1:-1].split(",")
                table, at = [{}], -1
                for op in ops[1:]:
                    k = body.index(op[:-1])
                    if k <= at:
                        table.append({})
                    table[-1][k], at = int(op[-1]), k
                assert len(table) <= 20, len(table)

                def step(i, carry, body=body, table=table):
                    late = body.index("F") if "F" in body else 0
                    stages(i, body, table, range(late))
                    since = min(n for n, row in enumerate(table) if max(row) >= late)
                    pl.when(i >= since)(lambda: stages(i, body, table, range(late, len(body))))
                    return carry

                def stages(i, body, table, ks):
                    for k in ks:
                        stage = body[k]
                        word = sum(row.get(k, 0) << (3 * n) for n, row in enumerate(table))
                        mask = sum((k in row) << n for n, row in enumerate(table))

                        @pl.when(((mask >> i) & 1) == 1)
                        def _():
                            for kind in stage:
                                run(kind + "+0", jnp.where(
                                    i < 10, (word & (2**30 - 1)) >> (3 * jnp.minimum(i, 9)),
                                    (word >> 30) >> (3 * jnp.maximum(i - 10, 0))) & 7)
                lax.fori_loop(0, len(table), step, 0)
            else:
                for op in ops:
                    run(op)


def make(**kw):
    cfg = dict(DEFAULT, **kw)
    cap = cfg["cap"]

    def kernel(x, router_W, route_idx, expert_W):
        dma = pltpu.SemaphoreType.DMA
        ri = route_idx.astype(I32).reshape(8, 128, 2).transpose(0, 2, 1).reshape(16, 128)
        x4 = x.reshape(128, 8, 4, 128).transpose(0, 2, 1, 3)
        return pl.pallas_call(
            functools.partial(_body, cfg),
            out_shape=jax.ShapeDtypeStruct((N_TOK, D_OUT), cfg.get("out_dtype", BF16)),
            in_specs=[pl.BlockSpec(memory_space=pl.ANY)] * 4,
            out_specs=pl.BlockSpec(memory_space=pltpu.VMEM),
            scratch_shapes=[
                pltpu.VMEM((N_EXP, D_IN), F32),
                pltpu.VMEM((16, 128), I32),
                pltpu.VMEM((2, 8, 128), I32),
                pltpu.SMEM((8, 128), I32),
                pltpu.SMEM((8, 128), I32),
                pltpu.VMEM((2, 8, 128), I32),
                pltpu.VMEM((NC, E_LOC, D_IN, CW), F32),
                *[pltpu.VMEM((4, YR, 128), F32)] * 4,
                pltpu.VMEM((E_LOC, 4, 4 * EW, 128), BF16),
                pltpu.VMEM((2, NG * 2 * cap, 128), BF16),
                pltpu.VMEM((2, NG * GS, 128), BF16),
                pltpu.VMEM((2, NG * GS, 128), BF16),
                pltpu.VMEM((2, N_TOK, 128), BF16),
                *[pltpu.VMEM((NC, 2, NG * cap, CW), BF16)] * 2,
                pltpu.VMEM((NB * HS, CW), F32),
                pltpu.VMEM((NC, N_DEV, NB * HS, CW), BF16),
                pltpu.VMEM((128, 4, 8, 128), F32),
                pltpu.VMEM((N_TOK, D_IN), BF16),
                pltpu.VMEM((E_LOC, N_TOK, CW), F32),
                pltpu.VMEM((NC, 4, N_TOK, CW), BF16),
                dma((NC + 3,)), dma((2,)), dma((2, NG, 20)), dma((NC,)),
                dma((NC, 2, 12)), dma((NC, 2, 3)), dma((NC, TB // cfg["fx"])),
            ],
            compiler_params=pltpu.CompilerParams(
                collective_id=0, vmem_limit_bytes=48 * 2**20,
                disable_semaphore_checks=cfg.get("nosem", True),
                disable_bounds_checks=cfg.get("nobounds", True)),
        )(x4, router_W.T, ri, expert_W)
    return kernel


def pallas_dist_moe_top2_ep_n1024_d512_e4_h1024_kernel(x, router_W, route_idx, expert_W):
    return make()(x, router_W, route_idx, expert_W)
```

```python
import functools

import jax
import jax.numpy as jnp
from jax import lax
from jax.experimental import pallas as pl
from jax.experimental.pallas import tpu as pltpu

N_TOK, D_IN, D_OUT = 1024, 512, 1024
N_DEV, E_LOC, N_EXP = 4, 4, 16
NB, TB, HS = 4, 256, 64
NG, GS = 2, 128
NC, CW = 8, 128
SENT, KEPT = 0, 1
EW = 64
YR = E_LOC * EW
CAP = 112
ALWAYS = (128, 104)
LIKELY = ((152, 160), (120, 120))
GROUP_PIECES = (52, 32, 16, 8, 4)
CHUNK_PIECES = (96, 64, 32, 16, 8, 4, 2)
FLEX, FX = (3, 4), 32
RELIEF = (16, 30)
LEAN_GAIN, LEAN_BIAS = (5, 7, 8, 7), (0, 24, 0, -24)

BF16, F32, I32 = jnp.bfloat16, jnp.float32, jnp.int32
MESH = pl.DeviceIdType.MESH


def _dot(a, b):
    return jnp.dot(a, b, preferred_element_type=F32)


def _dot_nt(a, b):
    return lax.dot_general(a, b, (((1,), (1,)), ((), ())), preferred_element_type=F32)


def _iota(shape, dim):
    return lax.broadcasted_iota(I32, shape, dim)


def _ones(mask):
    return jnp.where(mask, 1.0, 0.0)


def _aligned(i, n):
    return i if isinstance(i, int) else pl.multiple_of(i, n)


def _load(ref, rows):
    return jnp.concatenate([ref[j, rows, :] for j in range(ref.shape[0])], axis=1)


def _store(ref, rows, value):
    for j in range(ref.shape[0]):
        ref[j, rows, :] = value[:, j * 128:(j + 1) * 128].astype(ref.dtype)


def _apply(ref, first, n, rhs):
    return jnp.concatenate(
        [_dot(_load(ref, pl.ds(first + r, n // 2)), rhs) for r in (0, n // 2)], axis=0)


def _pick(idx, vals):
    out = vals[-1]
    for k in range(len(vals) - 2, -1, -1):
        out = jnp.where(idx == k, vals[k], out)
    return out


def _lanes(v, first=0, n=8):
    return jnp.concatenate([v[r:r + 1] for r in range(first, first + n)], axis=1)


def _widen(before, total, step):
    second = (_iota((8, 128), 0) & step) != 0
    prev, nxt = pltpu.roll(total, step, 0), pltpu.roll(total, 8 - step, 0)
    return before + jnp.where(second, prev, 0), total + jnp.where(second, prev, nxt)


def _count(flags):
    upper = _ones(_iota((128, 256), 0) < _iota((128, 256), 1)).astype(BF16)
    r = _dot(jnp.concatenate(flags, axis=0).astype(BF16), upper).astype(I32)
    return [_widen(r[8 * k:8 * k + 8, :128], r[8 * k:8 * k + 8, 128:], 1)
            for k in range(len(flags))]


def _starts(counts):
    out = [jnp.zeros((8, 128), I32)]
    for _, total in counts:
        out.append(out[-1] + total)
    return out


def _scatter(*parts):
    pos = jnp.concatenate([_lanes(p) for p, _ in parts], axis=1)
    n = pos.shape[1]
    hit = (pos >> 7) == _iota((8, n), 0)
    lhs = [jnp.where(hit, jnp.concatenate([_lanes(v) for v in vals], axis=1), 0).astype(F32)
           for vals in zip(*[v for _, v in parts])]
    if len(lhs) % 2:
        lhs.append(jnp.zeros((8, n), F32))
    out = _dot_nt(jnp.concatenate(lhs, axis=0).astype(BF16),
                  _ones((pos & 127) == _iota((128, n), 0)).astype(BF16)).astype(I32)
    return [out[8 * k:8 * k + 8] for k in range(len(parts[0][1]))]


def _homes(c0, c1, relief):
    sub = _iota((8, 128), 0)
    diff = (c1 - c0) & 3
    same, opposite = diff == 0, diff == 2
    lead = jnp.where(diff == 3, c1, c0)
    kind = jnp.where(same, c0, jnp.where(opposite, 8 + (c0 & 1), 4 + lead))
    rank, count = zip(*_count([_ones(kind == k) for k in range(10)]))
    s, a, o = count[:4], count[4:8], count[8:]
    parity = (sub >> 1) & 1
    d1 = jnp.clip((o[0] + s[1] - s[3] + parity) >> 1, 0, o[0])
    q0 = s[0] + a[0] - HS
    q1 = q0 + s[1] + a[1] + d1 - HS
    q2 = q1 + s[2] + a[2] + o[1] - HS
    d0 = (o[1] + s[0] - s[2] + parity - relief) >> 1
    d0 = jnp.maximum(d0, jnp.maximum(q2 - a[2], -a[3]) - jnp.minimum(q0, q1))
    d0 = jnp.minimum(d0, jnp.minimum(a[0] - q0, a[1] - q1) + jnp.minimum(q2, 0))
    d0 = jnp.clip(d0, 0, o[1])
    d = [d0, d1, o[1] - d0, o[0] - d1]
    off = [q0 + d0, q1 + d0, q2, jnp.zeros_like(q2)]
    lo = functools.reduce(jnp.maximum, [-v for v in off])
    hi = functools.reduce(jnp.minimum, [a[m] - off[m] for m in range(4)])
    even = (a[0] + a[1] + a[2] + a[3] - 2 * (off[0] + off[1] + off[2]) + 4) >> 3
    up = [jnp.minimum(jnp.maximum(even, lo), hi) + v for v in off]

    first = _pick(kind - 4, rank[4:]) < _pick(kind - 4, up + [d[1], d[2]])
    home = jnp.where(same, c0, jnp.where(
        opposite, (c0 & 1) + jnp.where(first, 1, 3), lead + jnp.where(first, 1, 0))) & 3
    right = [_widen(0, up[m] + d[(m + 1) & 3], 2)[1] for m in range(4)]
    left = [_widen(0, a[m] - up[m] + d[m], 2)[1] for m in range(4)]
    return home, lo > hi, right, left


def _moe_body(x_hbm, rw_hbm, ri_hbm, w_hbm, out_ref,
              rwv, riv, wv, plan_v, plan_s, idx_v, idx_s0, idx_s1, tab, xs0, xs1, xs2, xs3, xg,
              to_send, to_keep, to_add, to_order, sbuf, rbuf, kept1, fbuf,
              xv, xd, gate, part,
              w_sem, i_sem, x_sem, send_sem, reduce_sem, share_sem, relay_sem):
    xs = ((xs0, xs1), (xs2, xs3))
    idx_s = (idx_s0, idx_s1)
    me = lax.axis_index("i")
    nbr = ((me + 1) & 3, (me + 3) & 3)

    def cols(c):
        return pl.ds(_aligned(c * CW, CW), CW)

    def weights(c):
        return pltpu.make_async_copy(w_hbm.at[:, :, cols(c)], wv.at[c], w_sem.at[c])

    def weights1(i):
        es = (pl.ds(0, E_LOC - 1), pl.ds(E_LOC - 1, 1))[i]
        return pltpu.make_async_copy(w_hbm.at[es, :, cols(1)], wv.at[1, es],
                                     w_sem.at[(1, NC + 2)[i]])

    def indices(kind):
        return pltpu.make_async_copy(idx_v.at[kind], idx_s[kind], i_sem.at[kind])

    def remote(src, dst, c, recv_sem, chip):
        return pltpu.make_async_remote_copy(
            src, dst, send_sem.at[c], recv_sem, device_id=(chip,), device_id_type=MESH)

    ri_copy = pltpu.make_async_copy(ri_hbm, riv, w_sem.at[NC])
    rw_copy = pltpu.make_async_copy(rw_hbm, rwv, w_sem.at[NC + 1])
    ri_copy.start()
    rw_copy.start()
    for copy in (weights(0), weights1(0), weights1(1)):
        copy.start(priority=1)

    barrier = pltpu.get_barrier_semaphore()
    for chip in nbr:
        pl.semaphore_signal(barrier, inc=1, device_id=(chip,), device_id_type=MESH)

    for kind in (SENT, KEPT):
        for ref in xs[kind]:
            rest = YR - ALWAYS[kind]
            ref[:, pl.ds(ALWAYS[kind], rest), :] = jnp.zeros((4, rest, 128), F32)

    ri_copy.wait()
    e0 = riv[pl.ds(0, 8, stride=2), :] & (N_EXP - 1)
    e1 = riv[pl.ds(1, 8, stride=2), :] & (N_EXP - 1)
    c0, c1 = e0 >> 2, e1 >> 2
    sub = _iota((8, 128), 0)
    token = sub * 128 + _iota((8, 128), 1)
    group_base = (sub >> 2) * YR

    def on(chip):
        return (c0 == chip) | (c1 == chip)

    def list_rows(kind, *where):
        tile, row = _scatter(*[(pos, (token >> 3, token & 7)) for pos in where])
        idx_v[kind] = jnp.concatenate([tile & 127, row & 7], axis=0)
        indices(kind).start()

    def plan(relief):
        home, stuck, right, left = _homes(c0, c1, relief)
        sent = on(me) & (home != me)
        mine = jnp.where(c0 == me, e0, e1) & 3
        by_expert = [_widen(*bt, 2)
                     for bt in _count([_ones(sent & (mine == e)) for e in range(E_LOC)])]
        start = _starts(by_expert)
        rank = _pick(mine, [before for before, _ in by_expert])
        list_rows(SENT, jnp.where(sent, group_base + _pick(mine, start[:4]) + rank, -1))
        for k, v in enumerate([(home - me) & 3, rank] + start[1:]):
            plan_v[k] = v

        bad = jnp.where(stuck | (functools.reduce(jnp.maximum, right + left) > CAP - 2), 1, 0)
        bins = _iota((2 * N_EXP, N_TOK), 0)
        load = (_ones(_lanes(e0 + jnp.where(c0 == home, N_EXP, 0)) == bins)
                + _ones(_lanes(e1 + jnp.where(c1 == home, N_EXP, 0)) == bins))
        for g in range(NG):
            over = jnp.sum(load[:, g * 2 * TB:(g + 1) * 2 * TB], axis=1, keepdims=True) > EW
            for i in range(4):
                bad = bad | jnp.where(over[8 * i:8 * i + 8], 1, 0)
        for shift in (4, 2, 1):
            bad = bad | pltpu.roll(bad, shift, 0)
        plan_s[2] = bad[0, 0]

        lean = []
        for m in range(4):
            gap = left[m] - right[(m - 1) & 3]
            gap = ((gap + pltpu.roll(gap, 4, 0)) * LEAN_GAIN[m]) >> 3
            lean.append((gap + LEAN_BIAS[m] + 4) >> 3)
        for j, chip in enumerate(nbr):
            plan_s[j] = _pick(jnp.full((8, 128), chip, I32), lean)[0, 0]

    def attempt(i, _):
        @pl.when(plan_s[2] != 0)
        def _():
            pl.when(i > 0)(lambda: indices(SENT).wait())
            plan(jnp.where(sub < 4, *RELIEF) * (1 - i))

    plan_s[2] = 1
    lax.fori_loop(0, 2, attempt, None)
    sparse = plan_s[2] == 0
    rw_copy.wait()

    def router(xb, b0, b1):
        scores = _dot_nt(rwv[...].astype(BF16), xb)
        probs = jnp.exp(scores - jnp.max(scores, axis=0, keepdims=True))
        probs = probs / jnp.sum(probs, axis=0, keepdims=True)
        expert = _iota(scores.shape, 0)
        return (jnp.sum(jnp.where(expert == b0, probs, 0.0), axis=0, keepdims=True),
                jnp.sum(jnp.where(expert == b1, probs, 0.0), axis=0, keepdims=True))

    @pl.when(jnp.logical_not(sparse))
    def _():
        x_copy = pltpu.make_async_copy(x_hbm, xv, i_sem.at[KEPT])
        x_copy.start()
        indices(SENT).wait()
        x_copy.wait()
        for c in range(2, NC):
            weights(c).start(priority=1)

        def gates(r, _):
            rows = pl.ds(_aligned(r * 128, 128), 128)
            xb = jnp.concatenate([xv[pl.ds(r * 16, 16), j].reshape(128, 128) for j in range(4)],
                                 axis=1).astype(BF16)
            xd[rows, :] = xb
            b0, b1 = (riv[pl.ds(2 * r + k, 1), :] & (N_EXP - 1) for k in range(2))
            g0, g1 = router(xb, b0, b1)
            for e in range(E_LOC):
                g = (jnp.where(b0 == me * E_LOC + e, g0 / (g0 + g1), 0.0)
                     + jnp.where(b1 == me * E_LOC + e, g1 / (g0 + g1), 0.0))
                gate[e, rows, :] = jnp.broadcast_to(g, (128, 128)).T

        lax.fori_loop(0, N_TOK // 128, gates, None)
        weights1(0).wait()
        weights1(1).wait()
        pl.semaphore_wait(barrier, 2)

        def my_half(c):
            return ((me + 1 - (c & 1)) >> 1) & 1

        def swap(c, hop):
            chip = jnp.where(((c + hop) & 1) == 0, me ^ 1, 3 - me)
            src = 1 - my_half(c) if hop == 0 else 2 * hop + 1
            return remote(part.at[c, src], part.at[c, 2 * hop + 2], c, relay_sem.at[c, hop], chip)

        def step(i, _):
            @pl.when(i < NC)
            def _():
                pl.when(i != 1)(lambda: weights(i).wait())

                def block(b, _):
                    rows = pl.ds(_aligned(b * 128, 128), 128)
                    part[i, b >> 2, pl.ds(_aligned((b & 3) * 128, 128), 128), :] = sum(
                        gate[e, rows, :] * _dot(xd[rows, :], wv[i, e].astype(BF16))
                        for e in range(E_LOC)).astype(BF16)

                lax.fori_loop(0, N_TOK // 128, block, None)
                swap(i, 0).start()

            for hop in range(3):
                c = i - 2 * (hop + 1)

                @pl.when((c >= 0) & (c < NC))
                def _():
                    swap(c, hop).wait()
                    if hop < 2:
                        ours = part[c, my_half(c) if hop == 0 else 3].astype(F32)
                        part[c, 2 * hop + 3] = (ours + part[c, 2 * hop + 2].astype(F32)).astype(BF16)
                        swap(c, hop + 1).start()
                    else:
                        for k, half in ((5, my_half(c)), (6, 1 - my_half(c))):
                            rows = pl.ds(_aligned(half * (N_TOK // 2), N_TOK // 2), N_TOK // 2)
                            out_ref[rows, cols(c)] = part[c, k].astype(out_ref.dtype)

        lax.fori_loop(0, NC + 6, step, None)

    @pl.when(sparse)
    def _():
        rel, sent_rank = plan_v[0], plan_v[1]
        sent_start = [None] + [plan_v[2 + e] for e in range(E_LOC)]
        lean = [plan_s[0], plan_s[1]]
        lists = [on(me) & (rel == 1), on(me) & (rel == 3),
                 on(nbr[1]) & (rel == 0), on(nbr[0]) & (rel == 0)]
        kept = [(c0 == me) & (rel == 0), (c1 == me) & (rel == 0)]
        counts = _count(
            [_ones(rel == h) for h in range(4)] + [_ones(v) for v in lists]
            + [_ones(kept[0] & ((e0 & 3) == e)) + _ones(kept[1] & ((e1 & 3) == e))
               for e in range(E_LOC)])
        slot = _pick(rel, [before for before, _ in counts[:4]])
        counts = [_widen(*bt, 2) for bt in counts[4:]]
        list_row = [jnp.where(sub < 4, CAP - 1 - before, before) for before, _ in counts[:4]]
        length = [[total[4 * g, 0] for g in range(NG)] for _, total in counts[:4]]
        kept_start = _starts(counts[4:])
        before = [v for v, _ in counts[4:]]
        kept_rank = [_pick(e0 & 3, before), _pick(e1 & 3, before) + jnp.where(e0 == e1, 1, 0)]
        list_rows(KEPT, *[
            jnp.where(kept[k], group_base + _pick(e & 3, kept_start[:4]) + kept_rank[k], -1)
            for k, e in enumerate((e0, e1))])
        edge = [[[0, 0]] + [[v[4 * g, 0] for g in range(NG)] for v in start[1:]]
                for start in (sent_start, kept_start)]

        def reduce_tables():
            my_row = (sub & 2) * (HS // 2) + slot + 1
            target = jnp.where(
                rel == 0, my_row, jnp.where(rel == 1, list_row[0], CAP + list_row[1]) + 1)
            tab[0], tab[1] = _scatter(*[
                (jnp.where(c == me, group_base + (e & 3) * EW
                           + jnp.where(rel == 0, NG * YR + kept_rank[k], sent_rank), -1),
                 (target, other))
                for k, (c, e, other) in enumerate(((c0, e0, e1), (c1, e1, e0)))])
            (came,) = _scatter(*[
                (jnp.where(lists[2 + j], group_base + j * 128 + list_row[2 + j], -1), (my_row,))
                for j in range(2)])
            for g in range(NG):
                _store(to_add, pl.ds(g * GS, GS),
                       _ones(_lanes(came, 2 * g, 2) == _iota((GS, YR), 0) + 1))

        def order_table():
            (who,) = _scatter(((sub >> 1) * TB + rel * HS + slot, (token & (TB - 1),)))
            for b in range(NB):
                _store(to_order, pl.ds(b * TB, TB),
                       _ones(_lanes(who, 2 * b, 2) == _iota((TB, TB), 0)))

        def fetch(kind, g, first, n, run):
            p = g * YR + first
            for i in range(n):
                tile, row = (idx_s[kind][h + (p >> 7), (p & 127) + i] for h in (0, 8))
                pltpu.make_async_copy(
                    x_hbm.at[tile, :, pl.ds(row, 1), :],
                    xs[kind][g].at[:, pl.ds(first + i, 1), :], x_sem.at[kind, g, run]).start()

        def fetched(kind, g, first, n, run):
            dst = xs[kind][g].at[:, pl.ds(_aligned(first, 8), n), :]
            pltpu.make_async_copy(dst, dst, x_sem.at[kind, g, run]).wait()

        def likely(kind, g, action):
            action(kind, g, 0, ALWAYS[kind], 0)
            for i, first in enumerate(range(ALWAYS[kind], LIKELY[kind][g], 8)):
                pl.when(first < edge[kind][E_LOC][g])(
                    functools.partial(action, kind, g, first, 8, i + 1))

        def further(kind, g, action):
            done = (LIKELY[kind][g] - ALWAYS[kind]) // 8
            runs = jnp.maximum((edge[kind][E_LOC][g] - ALWAYS[kind] + 7) >> 3, done)
            lax.fori_loop(
                done, runs, lambda i, _: action(kind, g, ALWAYS[kind] + 8 * i, 8, i + 1), None)

        def await_x(kind, g):
            further(kind, g, fetched)
            likely(kind, g, fetched)

        def prepare(kind, g):
            rows = pl.ds((kind * NG + g) * EW, EW)
            for e in range(E_LOC):
                _store(xg.at[e], rows, _load(xs[kind][g], pl.ds(edge[kind][e][g], EW)))
            target, other = (_lanes(tab[i], 2 * (kind * NG + g), 2) for i in range(2))
            g0, g1 = router(jnp.concatenate([_load(xg.at[e], rows) for e in range(E_LOC)], axis=0),
                            me * E_LOC + _iota((1, YR), 1) // EW, other)
            ref, n = ((to_send, 2 * CAP), (to_keep, GS))[kind]
            _store(ref, pl.ds(g * n, n),
                   jnp.where(target == _iota((n, YR), 0) + 1, g0 / (g0 + g1), 0.0))

        def products(c, kind, gs, experts=range(E_LOC)):
            rows = pl.ds((kind * NG + gs[0]) * EW, len(gs) * EW)
            return [_dot(_load(xg.at[e], rows), wv[c, e].astype(BF16)).astype(BF16)
                    for e in experts]

        def by_group(y):
            return [jnp.concatenate([v[r:r + EW] for v in y], axis=0)
                    for r in range(0, y[0].shape[0], EW)]

        def pack(c, gs, y):
            for g, yg in zip(gs, by_group(y)):
                for j in range(2):
                    sbuf[c, j, pl.ds(g * CAP, CAP), :] = _dot(
                        _load(to_send, pl.ds((2 * g + j) * CAP, CAP)), yg).astype(BF16)

        def reduce(c, gs, action):
            sizes = CHUNK_PIECES if len(gs) == NG else GROUP_PIECES
            unit = sizes[-1]
            at, stop = [], []
            for n0, n1 in length[2:] if action == "recv" else length[:2]:
                stop.append(CAP + n1 if 1 in gs else CAP)
                at.append((CAP - n0) & -unit if 0 in gs else CAP)
                if 1 not in gs:
                    at[-1] = jnp.minimum(at[-1], CAP - sizes[0])

            def piece(j, i, first):
                rows = pl.ds(_aligned(first, unit), sizes[i])
                do(action, remote(sbuf.at[c, j, rows], rbuf.at[c, j, rows], c,
                                  reduce_sem.at[c, j, gs[0] * len(sizes) + i], nbr[j]))

            for i, n in enumerate(sizes):
                for j in range(2):
                    if i == 0:
                        piece(j, i, at[j])
                        at[j] = at[j] + n
                    else:
                        needed = at[j] + n < stop[j] + unit
                        pl.when(needed)(functools.partial(piece, j, i, at[j]))
                        at[j] = at[j] + jnp.where(needed, n, 0)

        def arrived(c, g):
            r = _iota((CAP, CW), 0)
            got = []
            for j in range(2):
                used = r >= CAP - length[2 + j][0] if g == 0 else r < length[2 + j][1]
                got += [jnp.where(used, rbuf[c, j, pl.ds(g * CAP, CAP), :].astype(F32), 0.0),
                        jnp.zeros((128 - CAP, CW), F32)]
            return _apply(to_add, g * GS, GS, jnp.concatenate(got, axis=0).astype(BF16))

        def finish(c, gs, y):
            for g, yg in zip(gs, by_group(y)):
                fbuf[c, 0, pl.ds(g * GS, GS), :] = (
                    arrived(c, g) + _apply(to_keep, g * GS, GS, yg)).astype(BF16)

        def share(c, j, b, n=2):
            rows = pl.ds(b * HS, n * HS)
            return remote(fbuf.at[c, 0, rows], fbuf.at[c, 3 - 2 * j, rows], c,
                          share_sem.at[c, j, (b + 2 * j + 2) & 3], nbr[j])

        def relay(c, j, first, n):
            rows = pl.ds(first, n)
            return remote(fbuf.at[c, 3 - 2 * j, rows], fbuf.at[c, 2, rows], c,
                          relay_sem.at[c, first // FX], nbr[j])

        def last_hop(c, j, b, n):
            return relay(c, j, b * HS, n * HS) if b // 2 == j else share(c, j, b, n)

        def do(action, copy):
            if action == "start":
                copy.start()
            elif action == "recv":
                copy.wait_recv()
            else:
                copy.wait_send()

        def share_rest(c):
            for j in (1, 0):
                share(c, j, 2 - 2 * j).start()

        def relay_halves(c):
            for j in range(2):
                share(c, j, 2 * j).wait_recv()
                relay(c, j, j * GS, GS).start()

        def relay_leaning(c, action):
            half = GS // FX
            later = (FLEX[-1] - c) * half
            for i in range(2 * half):
                for j in range(2):
                    split = half + jnp.where(lean[j] > 0, jnp.maximum(lean[j] - later, 0),
                                             jnp.minimum(lean[j] + later, 0))
                    pl.when(i < split if j == 0 else i >= split)(
                        lambda: do(action, relay(c, j, i * FX, FX)))

        def await_halves(c):
            for b in (0, 2):
                for j in range(2):
                    last_hop(c, j, b, 2).wait()

        def await_first_sends(c, groupings):
            for gs in groupings:
                reduce(c, gs, "sent")
            for j in range(2):
                share(c, j, 2 * j).wait_send()

        def write(c, b):
            rows = jnp.concatenate([fbuf[c, h, pl.ds(b * HS, HS), :] for h in range(4)], axis=0)
            out_ref[pl.ds(b * TB, TB), cols(c)] = _apply(
                to_order, b * TB, TB, rows).astype(out_ref.dtype)

        both = (0, 1)
        indices(SENT).wait()
        likely(SENT, 0, fetch)
        reduce_tables()
        further(SENT, 0, fetch)
        likely(SENT, 1, fetch)
        order_table()
        further(SENT, 1, fetch)
        indices(KEPT).wait()
        pl.semaphore_wait(barrier, 2)
        weights(0).wait()
        for g in both:
            await_x(SENT, g)
            prepare(SENT, g)
            pack(0, (g,), products(0, SENT, (g,)))
            reduce(0, (g,), "start")
        further(KEPT, 0, fetch)
        weights1(0).wait()
        likely(KEPT, 0, fetch)
        y = products(1, SENT, both, range(E_LOC - 1))
        further(KEPT, 1, fetch)
        weights1(1).wait()
        likely(KEPT, 1, fetch)
        pack(1, both, y + products(1, SENT, both, [E_LOC - 1]))
        reduce(1, (0,), "start")
        for c in range(2, NC):
            weights(c).start(priority=1)
        for g in both:
            await_x(KEPT, g)
            if g == 0:
                reduce(1, (1,), "start")
            prepare(KEPT, g)
            y = products(0, KEPT, (g,))
            reduce(0, (g,), "recv")
            finish(0, (g,), y)
            for j in (g, 1 - g):
                share(0, j, 2 * g).start()
        for g, yg in enumerate(by_group(products(1, KEPT, both))):
            kept1[pl.ds(g * GS, GS), :] = _apply(to_keep, g * GS, GS, yg)
        for g in both:
            rows = pl.ds(g * GS, GS)
            reduce(1, (g,), "recv")
            fbuf[1, 0, rows, :] = (kept1[rows, :] + arrived(1, g)).astype(BF16)
            for j in (g, 1 - g):
                share(1, j, 2 * g).start()

        def produce(i, _):
            @pl.when(i < NC)
            def _():
                weights(i).wait()
                pack(i, both, products(i, SENT, both))
                reduce(i, both, "start")

            @pl.when(i >= 4)
            def _():
                reduce(i - 2, both, "recv")
                finish(i - 2, both, products(i - 2, KEPT, both))
                for j in range(2):
                    share(i - 2, j, 2 * j).start()

            pl.when((i >= 4) & (i < NC))(lambda: share_rest(i - 2))
            pl.when((i < 4) | (i == 7))(lambda: relay_halves(jnp.minimum(i - 2, 2)))

            @pl.when((i == 7) | (i == 8))
            def _():
                for j in range(2):
                    for b in (0, 2):
                        share(i - 4, j, b).wait_recv()
                relay_leaning(i - 4, "start")
                await_halves(i - 7)
                await_first_sends(i - 7, ((0,), (1,)))
                for b in range(NB):
                    write(i - 7, b)

        lax.fori_loop(2, NC + 2, produce, None)
        relay_halves(5)
        share_rest(6)

        def collect(c, _):
            pl.when(c == 3)(lambda: relay_halves(6))

            @pl.when(c == 4)
            def _():
                for j in range(2):
                    share(NC - 1, j, 2 * j).wait_recv()
                for b in range(NB):
                    for j in range(2):
                        last_hop(NC - 1, j, b, 1).start()

            leaning = (c >= FLEX[0]) & (c <= FLEX[-1])

            @pl.when(leaning)
            def _():
                for j in range(2):
                    share(c, j, 2 - 2 * j).wait_send()
                relay_leaning(c, "sent")
                for first in range(0, TB, FX):
                    relay(c, 0, first, FX).wait_recv()

            pl.when(jnp.logical_not(leaning))(lambda: await_halves(c))
            await_first_sends(c, (both,))
            for b in range(NB):
                write(c, b)

        lax.fori_loop(2, NC - 1, collect, None)
        await_first_sends(NC - 1, (both,))
        for b in range(NB):
            for j in range(2):
                last_hop(NC - 1, j, b, 1).wait_recv()
            write(NC - 1, b)
        for b in range(NB):
            for j in range(2):
                last_hop(NC - 1, j, b, 1).wait_send()


def pallas_dist_moe_top2_ep_n1024_d512_e4_h1024_kernel(
    x: jax.Array,
    router_W: jax.Array,
    route_idx: jax.Array,
    expert_W: jax.Array,
):
    dma = pltpu.SemaphoreType.DMA
    x_tiles = x.reshape(N_TOK // 8, 8, D_IN // 128, 128).transpose(0, 2, 1, 3)
    routes = route_idx.astype(I32).reshape(8, 128, 2).transpose(0, 2, 1).reshape(16, 128)
    return pl.pallas_call(
        _moe_body,
        out_shape=jax.ShapeDtypeStruct((N_TOK, D_OUT), BF16),
        in_specs=[pl.BlockSpec(memory_space=pl.ANY)] * 4,
        out_specs=pl.BlockSpec(memory_space=pltpu.VMEM),
        scratch_shapes=[
            pltpu.VMEM((N_EXP, D_IN), F32),
            pltpu.VMEM((16, 128), I32),
            pltpu.VMEM((NC, E_LOC, D_IN, CW), F32),
            pltpu.VMEM((2 + E_LOC, 8, 128), I32),
            pltpu.SMEM((3,), I32),
            pltpu.VMEM((2, 16, 128), I32),
            *[pltpu.SMEM((16, 128), I32)] * 2,
            pltpu.VMEM((2, 8, 128), I32),
            *[pltpu.VMEM((4, YR, 128), F32)] * 4,
            pltpu.VMEM((E_LOC, 4, 2 * NG * EW, 128), BF16),
            pltpu.VMEM((2, NG * 2 * CAP, 128), BF16),
            *[pltpu.VMEM((2, NG * GS, 128), BF16)] * 2,
            pltpu.VMEM((2, N_TOK, 128), BF16),
            *[pltpu.VMEM((NC, 2, NG * CAP, CW), BF16)] * 2,
            pltpu.VMEM((NG * GS, CW), F32),
            pltpu.VMEM((NC, N_DEV, NG * GS, CW), BF16),
            pltpu.VMEM((N_TOK // 8, 4, 8, 128), F32),
            pltpu.VMEM((N_TOK, D_IN), BF16),
            pltpu.VMEM((E_LOC, N_TOK, CW), F32),
            pltpu.VMEM((NC, 7, N_TOK // 2, CW), BF16),
            dma((NC + 3,)),
            dma((2,)),
            dma((2, NG, 1 + (YR - min(ALWAYS)) // 8)),
            dma((NC,)),
            dma((NC, 2, NG * len(GROUP_PIECES))),
            dma((NC, 2, 3)),
            dma((NC, TB // FX)),
        ],
        compiler_params=pltpu.CompilerParams(
            collective_id=0,
            vmem_limit_bytes=48 * 2**20,
            disable_bounds_checks=True,
            disable_semaphore_checks=True,
        ),
    )(x_tiles, router_W.T, routes, expert_W)
```
